```python
import numpy as np

kernel_name = "dist_mean_ax0_xy_m1024_n512"

def setup_inputs():
    return {"x": np.random.randn(2048, 1024).astype(np.float32)}

def reference(x: np.ndarray) -> np.ndarray:
    return np.mean(x, axis=0, keepdims=True)
```

```python
import jax
import jax.numpy as jnp
from jax import lax
from jax.experimental import pallas as pl
from jax.experimental.pallas import tpu as pltpu

_N_CHUNKS = 4


def pallas_dist_mean_ax0_xy_m1024_n512_kernel(
x: jax.Array,
):
    m, n = x.shape
    n_x = 2
    rows = m // _N_CHUNKS
    inv_rows = 1.0 / (m * n_x)

    def kernel_body(x_hbm, out_ref, xbuf, send_buf, recv_buf,
                    load_sems, send_sem, recv_sem):
        my_x = lax.axis_index("x")
        my_y = lax.axis_index("y")
        nbr = (1 - my_x, my_y)

        loads = [
            pltpu.make_async_copy(
                x_hbm.at[pl.ds(i * rows, rows)],
                xbuf.at[pl.ds(i * rows, rows)],
                load_sems.at[i],
            )
            for i in range(_N_CHUNKS)
        ]
        for c in loads:
            c.start()

        barrier = pltpu.get_barrier_semaphore()
        pl.semaphore_signal(barrier, inc=1, device_id=nbr,
                            device_id_type=pl.DeviceIdType.MESH)

        acc = None
        for i, c in enumerate(loads):
            c.wait()
            chunk = xbuf[pl.ds(i * rows, rows), :]
            part = jnp.sum(chunk.reshape(rows // 8, 8, n), axis=0)
            acc = part if acc is None else acc + part
        mine = jnp.sum(acc, axis=0, keepdims=True)
        send_buf[...] = mine

        pl.semaphore_wait(barrier, 1)
        rdma = pltpu.make_async_remote_copy(
            src_ref=send_buf,
            dst_ref=recv_buf,
            send_sem=send_sem,
            recv_sem=recv_sem,
            device_id=nbr,
            device_id_type=pl.DeviceIdType.MESH,
        )
        rdma.start()
        rdma.wait()
        out_ref[...] = (mine + recv_buf[...]) * inv_rows

    return pl.pallas_call(
        kernel_body,
        out_shape=jax.ShapeDtypeStruct((1, n), x.dtype),
        in_specs=[pl.BlockSpec(memory_space=pl.ANY)],
        out_specs=pl.BlockSpec(memory_space=pltpu.VMEM),
        scratch_shapes=[
            pltpu.VMEM((m, n), x.dtype),
            pltpu.VMEM((1, n), jnp.float32),
            pltpu.VMEM((1, n), jnp.float32),
            pltpu.SemaphoreType.DMA((_N_CHUNKS,)),
            pltpu.SemaphoreType.DMA,
            pltpu.SemaphoreType.DMA,
        ],
        compiler_params=pltpu.CompilerParams(collective_id=0),
    )(x)
```

```python
import jax
import jax.numpy as jnp
from jax import lax
from jax.experimental import pallas as pl
from jax.experimental.pallas import tpu as pltpu

_X_SIZE = 2

_CHUNK_32NDS = (28, 3, 1)


def pallas_dist_mean_ax0_xy_m1024_n512_kernel(
x: jax.Array,
):
    m, n = x.shape
    assert m % (32 * 8) == 0, "row chunks must be whole (8, 128) tiles"
    rows = [m // 32 * c for c in _CHUNK_32NDS]
    offs = [sum(rows[:i]) for i in range(len(rows))]
    inv_rows = 1.0 / (m * _X_SIZE)

    def kernel_body(x_hbm, out_ref, xbuf, send_buf, recv_buf,
                    load_sems, send_sem, recv_sem):
        my_x = lax.axis_index("x")
        my_y = lax.axis_index("y")
        nbr = (1 - my_x, my_y)

        loads = [
            pltpu.make_async_copy(
                x_hbm.at[pl.ds(o, r)], xbuf.at[pl.ds(o, r)], load_sems.at[i]
            )
            for i, (o, r) in enumerate(zip(offs, rows))
        ]
        for c in loads:
            c.start()

        barrier = pltpu.get_barrier_semaphore()
        pl.semaphore_signal(barrier, inc=1, device_id=nbr,
                            device_id_type=pl.DeviceIdType.MESH)

        acc = None
        for i, c in enumerate(loads):
            if i == 1:
                pl.semaphore_wait(barrier, 1)
            c.wait()
            chunk = xbuf[pl.ds(offs[i], rows[i]), :]
            part = jnp.sum(chunk.reshape(rows[i] // 8, 8, n), axis=0)
            acc = part if acc is None else acc + part
        mine = jnp.sum(acc, axis=0, keepdims=True)

        send_buf[...] = mine
        rdma = pltpu.make_async_remote_copy(
            src_ref=send_buf,
            dst_ref=recv_buf,
            send_sem=send_sem,
            recv_sem=recv_sem,
            device_id=nbr,
            device_id_type=pl.DeviceIdType.MESH,
        )
        rdma.start()
        rdma.wait_recv()
        out_ref[...] = ((mine + recv_buf[...]) * inv_rows).astype(out_ref.dtype)
        rdma.wait_send()

    return pl.pallas_call(
        kernel_body,
        out_shape=jax.ShapeDtypeStruct((1, n), x.dtype),
        in_specs=[pl.BlockSpec(memory_space=pl.ANY)],
        out_specs=pl.BlockSpec(memory_space=pltpu.VMEM),
        scratch_shapes=[
            pltpu.VMEM((m, n), x.dtype),
            pltpu.VMEM((1, n), jnp.float32),
            pltpu.VMEM((1, n), jnp.float32),
            pltpu.SemaphoreType.DMA((len(rows),)),
            pltpu.SemaphoreType.DMA,
            pltpu.SemaphoreType.DMA,
        ],
        compiler_params=pltpu.CompilerParams(
            collective_id=0,
            disable_semaphore_checks=True,
        ),
    )(x)
```
